```python
import numpy as np

kernel_name = "dist_mean_ax1_xy_m1024_n512"

def setup_inputs():
    return {"x": np.random.randn(2048, 1024).astype(np.float32)}

def reference(x: np.ndarray) -> np.ndarray:
    return np.mean(x, axis=1, keepdims=True)
```

```python
import jax
import jax.numpy as jnp
from jax import lax
from jax.experimental import pallas as pl
from jax.experimental.pallas import tpu as pltpu

_SUBLANES, _LANES = 8, 128
_ROWS, _COLS = 1024, 512

_SPLIT, _BLOCK_ROWS, _BLOCK_SPREAD = 768, 16, 0.65
_SEGMENTS = (
    ((0, 128),),
    ((128, 128), (768, 128)),
    ((256, 128),),
    ((384, 128), (896, 128)),
    ((512, 144),),
    ((656, 72),),
    ((728, 40),),
)
_LAG = 135


def _load_plan():
    tiles = [
        (r, _SUBLANES, c, _LANES, 1)
        for r in range(0, _SPLIT, _SUBLANES)
        for c in range(0, _COLS, _LANES)
    ]
    blocks = [(r, _BLOCK_ROWS, 0, _COLS, 0) for r in range(_SPLIT, _ROWS, _BLOCK_ROWS)]
    timed = [(_BLOCK_SPREAD * (i + 0.5) / len(blocks), b) for i, b in enumerate(blocks)]
    timed += [((i + 0.5) / len(tiles), t) for i, t in enumerate(tiles)]
    return [copy for _, copy in sorted(timed, key=lambda entry: entry[0])]


def _locate(row):
    for segment, ranges in enumerate(_SEGMENTS):
        offset = 0
        for first, count in ranges:
            if first <= row < first + count:
                return segment, offset + row - first
            offset += count
    raise ValueError(f"row {row} is in no segment")


def pallas_dist_mean_ax1_xy_m1024_n512_kernel(
x: jax.Array,
):
    assert x.shape == (_ROWS, _COLS), x.shape
    scale = 1.0 / (2 * _COLS)
    groups = _ROWS // _LANES
    plan = _load_plan()
    last = len(_SEGMENTS) - 1
    ((last_row, last_count),) = _SEGMENTS[last]
    tail = last_row // _LANES
    reduce_after = [0] * len(_SEGMENTS)
    for started, (row, *_) in enumerate(plan, 1):
        reduce_after[_locate(row)[0]] = started + _LAG

    def kernel_body(x_ref, o_ref, bufs, early_src, early_dst, late_src, late_dst,
                    last_src, last_dst, load_sems, send_sems, recv_sems):
        shape = (_SUBLANES, _LANES)
        diagonal = (lax.broadcasted_iota(jnp.int32, shape, 1)
                    - lax.broadcasted_iota(jnp.int32, shape, 0))
        zeros = jnp.zeros(shape, jnp.float32)
        tiles = [zeros] * groups
        missing = [_LANES] * groups

        def row_sums(segment):
            buf = bufs[segment]
            pltpu.make_async_copy(buf, buf, load_sems.at[segment]).wait()
            sums = []
            for first, count in _SEGMENTS[segment]:
                for row in range(first, first + count, _SUBLANES):
                    rows = pl.ds(_locate(row)[1], _SUBLANES)
                    parts = [buf[rows, pl.ds(c, _LANES)] for c in range(0, _COLS, _LANES)]
                    while len(parts) > 1:
                        parts = [a + b for a, b in zip(parts[::2], parts[1::2])]
                    sums.append((row, jnp.sum(parts[0], axis=1, keepdims=True)))
            return sums

        def exchange(src, dst, i):
            return pltpu.make_async_remote_copy(
                src, dst, send_sems.at[i], recv_sems.at[i],
                device_id=peer, device_id_type=pl.DeviceIdType.MESH,
            )

        def reduce(segment):
            completed = False
            for row, sums in row_sums(segment):
                g = row // _LANES
                tiles[g] = jnp.where(diagonal == row % _LANES, sums, tiles[g])
                missing[g] -= _SUBLANES
                if missing[g] == 0:
                    slot = g if g < tail else g - 1
                    early_src[pl.ds(slot, 1), :] = jnp.sum(tiles[g], axis=0, keepdims=True)
                    completed = True
            if completed and sum(missing) == missing[tail]:
                pl.semaphore_wait(barrier, 1)
                exchange(early_src, early_dst, 0).start()

        reduced = 0
        for started, (row, rows, col, cols, priority) in enumerate(plan, 1):
            segment, offset = _locate(row)
            pltpu.make_async_copy(
                x_ref.at[pl.ds(row, rows), pl.ds(col, cols)],
                bufs[segment].at[pl.ds(offset, rows), pl.ds(col, cols)],
                load_sems.at[segment],
            ).start(priority=priority)
            if started == 64:
                peer = (lax.axis_index("x"), 1 - lax.axis_index("y"))
                barrier = pltpu.get_barrier_semaphore()
                pl.semaphore_signal(
                    barrier, 1, device_id=peer, device_id_type=pl.DeviceIdType.MESH
                )
            while reduced < last and reduce_after[reduced] <= started:
                reduce(reduced)
                reduced += 1
        for segment in range(reduced, last):
            reduce(segment)

        early = exchange(early_src, early_dst, 0)
        late = exchange(late_src, late_dst, 1)
        final = exchange(last_src, last_dst, 2)
        last_sums = row_sums(last)
        late_row = jnp.sum(tiles[tail], axis=0, keepdims=True)
        late_src[...] = late_row
        late.start()
        tile = zeros
        for row, sums in last_sums:
            tile = jnp.where(diagonal == row % _LANES, sums, tile)
        final_row = jnp.sum(tile, axis=0, keepdims=True)
        last_src[...] = final_row
        final.start()

        early.wait_send()
        late.wait_send()
        final.wait_send()
        early.wait_recv()
        means = (early_src[...] + early_dst[...]) * scale
        o_ref[pl.ds(0, tail), :] = means[:tail]
        o_ref[pl.ds(tail + 1, groups - tail - 1), :] = means[tail:]
        late.wait_recv()
        total = (late_row + final_row) + late_dst[...]
        lane = lax.broadcasted_iota(jnp.int32, (1, _LANES), 1)
        final.wait_recv()
        theirs = jnp.zeros((1, _LANES), jnp.float32)
        for i in range(last_row % _LANES, last_row % _LANES + last_count):
            theirs = jnp.where(lane == i, last_dst[0, i], theirs)
        o_ref[pl.ds(tail, 1), :] = (total + theirs) * scale

    def vmem(rows, cols=_LANES):
        return pltpu.VMEM((rows, cols), jnp.float32)

    out = pl.pallas_call(
        kernel_body,
        out_shape=vmem(groups),
        in_specs=[pl.BlockSpec(memory_space=pltpu.HBM)],
        out_specs=pl.BlockSpec(memory_space=pltpu.VMEM),
        scratch_shapes=[
            [vmem(sum(count for _, count in ranges), _COLS) for ranges in _SEGMENTS],
            vmem(groups - 1), vmem(groups - 1),
            vmem(1), vmem(1),
            vmem(1), pltpu.SMEM((1, _LANES), jnp.float32),
            pltpu.SemaphoreType.DMA((len(_SEGMENTS),)),
            pltpu.SemaphoreType.DMA((3,)),
            pltpu.SemaphoreType.DMA((3,)),
        ],
        compiler_params=pltpu.CompilerParams(
            collective_id=0, disable_semaphore_checks=True
        ),
    )(x)
    return out.reshape(_ROWS, 1)
```

```python
import jax
import jax.numpy as jnp
from jax import lax
from jax.experimental import pallas as pl
from jax.experimental.pallas import tpu as pltpu

_SUBLANES, _LANES = 8, 128
_ROWS, _COLS = 1024, 512

_SPLIT, _BLOCK_ROWS, _BLOCK_SPREAD = 768, 16, 0.65
_SEGMENTS = (
    ((0, 128),),
    ((128, 128), (768, 128)),
    ((256, 128),),
    ((384, 128), (896, 128)),
    ((512, 144),),
    ((656, 72),),
    ((728, 40),),
)
_LAG = 135


def _load_plan():
    tiles = [
        (r, _SUBLANES, c, _LANES, 1)
        for r in range(0, _SPLIT, _SUBLANES)
        for c in range(0, _COLS, _LANES)
    ]
    blocks = [(r, _BLOCK_ROWS, 0, _COLS, 0) for r in range(_SPLIT, _ROWS, _BLOCK_ROWS)]
    timed = [(_BLOCK_SPREAD * (i + 0.5) / len(blocks), b) for i, b in enumerate(blocks)]
    timed += [((i + 0.5) / len(tiles), t) for i, t in enumerate(tiles)]
    return [copy for _, copy in sorted(timed, key=lambda entry: entry[0])]


def _locate(row):
    for segment, ranges in enumerate(_SEGMENTS):
        offset = 0
        for first, count in ranges:
            if first <= row < first + count:
                return segment, offset + row - first
            offset += count
    raise ValueError(f"row {row} is in no segment")


def pallas_dist_mean_ax1_xy_m1024_n512_kernel(
x: jax.Array,
):
    assert x.shape == (_ROWS, _COLS), x.shape
    scale = 1.0 / (2 * _COLS)
    groups = _ROWS // _LANES
    plan = _load_plan()
    last = len(_SEGMENTS) - 1
    ((last_row, last_count),) = _SEGMENTS[last]
    tail = last_row // _LANES
    reduce_after = [0] * len(_SEGMENTS)
    for count, (row, *_) in enumerate(plan, 1):
        reduce_after[_locate(row)[0]] = count + _LAG

    def kernel_body(x_ref, o_ref, bufs, early_src, early_dst, late_src, late_dst,
                    last_src, last_dst, load_sems, send_sems, recv_sems):
        started = 0

        def load_until(count):
            nonlocal started
            for row, rows, col, cols, priority in plan[started:count]:
                segment, offset = _locate(row)
                pltpu.make_async_copy(
                    x_ref.at[pl.ds(row, rows), pl.ds(col, cols)],
                    bufs[segment].at[pl.ds(offset, rows), pl.ds(col, cols)],
                    load_sems.at[segment],
                ).start(priority=priority)
            started = max(started, count)

        def row_sums(segment):
            buf = bufs[segment]
            pltpu.make_async_copy(buf, buf, load_sems.at[segment]).wait()
            sums = []
            for first, count in _SEGMENTS[segment]:
                for row in range(first, first + count, _SUBLANES):
                    rows = pl.ds(_locate(row)[1], _SUBLANES)
                    parts = [buf[rows, pl.ds(c, _LANES)] for c in range(0, _COLS, _LANES)]
                    while len(parts) > 1:
                        parts = [a + b for a, b in zip(parts[::2], parts[1::2])]
                    sums.append((row, jnp.sum(parts[0], axis=1, keepdims=True)))
            return sums

        load_until(64)
        peer = (lax.axis_index("x"), 1 - lax.axis_index("y"))
        barrier = pltpu.get_barrier_semaphore()
        pl.semaphore_signal(barrier, 1, device_id=peer, device_id_type=pl.DeviceIdType.MESH)
        early, late, final = (
            pltpu.make_async_remote_copy(
                src, dst, send_sems.at[i], recv_sems.at[i],
                device_id=peer, device_id_type=pl.DeviceIdType.MESH,
            )
            for i, (src, dst) in enumerate(
                ((early_src, early_dst), (late_src, late_dst), (last_src, last_dst))
            )
        )

        shape = (_SUBLANES, _LANES)
        diagonal = (lax.broadcasted_iota(jnp.int32, shape, 1)
                    - lax.broadcasted_iota(jnp.int32, shape, 0))
        zeros = jnp.zeros(shape, jnp.float32)
        tiles = [zeros] * groups
        missing = [_LANES] * groups
        for segment in range(last):
            load_until(reduce_after[segment])
            for row, sums in row_sums(segment):
                g = row // _LANES
                tiles[g] = jnp.where(diagonal == row % _LANES, sums, tiles[g])
                missing[g] -= _SUBLANES
                if missing[g] == 0:
                    slot = g if g < tail else g - 1
                    early_src[pl.ds(slot, 1), :] = jnp.sum(tiles[g], axis=0, keepdims=True)
                    if sum(missing) == missing[tail]:
                        pl.semaphore_wait(barrier, 1)
                        early.start()
        load_until(len(plan))

        last_sums = row_sums(last)
        late_row = jnp.sum(tiles[tail], axis=0, keepdims=True)
        late_src[...] = late_row
        late.start()
        tile = zeros
        for row, sums in last_sums:
            tile = jnp.where(diagonal == row % _LANES, sums, tile)
        final_row = jnp.sum(tile, axis=0, keepdims=True)
        last_src[...] = final_row
        final.start()

        early.wait_send()
        late.wait_send()
        final.wait_send()
        early.wait_recv()
        means = (early_src[...] + early_dst[...]) * scale
        o_ref[pl.ds(0, tail), :] = means[:tail]
        o_ref[pl.ds(tail + 1, groups - tail - 1), :] = means[tail:]
        late.wait_recv()
        total = (late_row + final_row) + late_dst[...]
        lane = lax.broadcasted_iota(jnp.int32, (1, _LANES), 1)
        final.wait_recv()
        theirs = jnp.zeros((1, _LANES), jnp.float32)
        for i in range(last_row % _LANES, last_row % _LANES + last_count):
            theirs = jnp.where(lane == i, last_dst[0, i], theirs)
        o_ref[pl.ds(tail, 1), :] = (total + theirs) * scale

    def vmem(rows, cols=_LANES):
        return pltpu.VMEM((rows, cols), jnp.float32)

    out = pl.pallas_call(
        kernel_body,
        out_shape=vmem(groups),
        in_specs=[pl.BlockSpec(memory_space=pltpu.HBM)],
        out_specs=pl.BlockSpec(memory_space=pltpu.VMEM),
        scratch_shapes=[
            [vmem(sum(count for _, count in ranges), _COLS) for ranges in _SEGMENTS],
            vmem(groups - 1), vmem(groups - 1),
            vmem(1), vmem(1),
            vmem(1), pltpu.SMEM((1, _LANES), jnp.float32),
            pltpu.SemaphoreType.DMA((len(_SEGMENTS),)),
            pltpu.SemaphoreType.DMA((3,)),
            pltpu.SemaphoreType.DMA((3,)),
        ],
        compiler_params=pltpu.CompilerParams(
            collective_id=0, disable_semaphore_checks=True
        ),
    )(x)
    return out.reshape(_ROWS, 1)
```
